```python
import numpy as np

kernel_name = "dist_mean_ax1_xy_m1024_n512"

def setup_inputs():
    return {"x": np.random.randn(2048, 1024).astype(np.float32)}

def reference(x: np.ndarray) -> np.ndarray:
    return np.mean(x, axis=1, keepdims=True)
```

```python
import jax
import jax.numpy as jnp
from jax import lax
from jax.experimental import pallas as pl
from jax.experimental.pallas import tpu as pltpu

_LANES = 128
_SUBLANES = 8
_Y_SIZE = 2
_DETOUR_ROWS = 24
_TAIL_ROWS = 48


def pallas_dist_mean_ax1_xy_m1024_n512_kernel(x: jax.Array):
    m, n = x.shape
    groups = m // _LANES
    scale = 1.0 / (_Y_SIZE * n)
    cuts = [_DETOUR_ROWS, *range(_LANES, m, _LANES), m - _TAIL_ROWS, m]
    chunks = list(zip(cuts[:-1], cuts[1:]))

    def body(x_hbm, out_ref, xv, hop, part, tail, recv, recv_tail,
             load_sems, hop_sems, send_sems, recv_sems):
        loads = [
            pltpu.make_async_copy(
                x_hbm.at[pl.ds(lo, hi - lo)], xv.at[pl.ds(lo, hi - lo)], load_sems.at[i]
            )
            for i, (lo, hi) in enumerate(chunks)
        ]
        hop_in = pltpu.make_async_copy(
            x_hbm.at[pl.ds(0, _DETOUR_ROWS)], hop, hop_sems.at[0]
        )
        hop_out = pltpu.make_async_copy(
            hop, xv.at[pl.ds(0, _DETOUR_ROWS)], hop_sems.at[1]
        )
        loads[0].start()
        hop_in.start()
        for load in loads[1:]:
            load.start()

        peer = (lax.axis_index("x"), 1 - lax.axis_index("y"))
        barrier = pltpu.get_barrier_semaphore()
        pl.semaphore_signal(
            barrier, 1, device_id=peer, device_id_type=pl.DeviceIdType.MESH
        )

        def remote(i, src, dst):
            return pltpu.make_async_remote_copy(
                src, dst, send_sems.at[i], recv_sems.at[i],
                device_id=peer, device_id_type=pl.DeviceIdType.MESH,
            )

        head = pl.ds(0, groups - 1)
        last = pl.ds(groups - 1, 1)
        msg_head = remote(0, part.at[head], recv.at[head])
        msg_last = remote(1, part.at[last], recv.at[last])
        msg_tail = remote(2, tail, recv_tail)

        tile = (_SUBLANES, _LANES)
        diag = lax.broadcasted_iota(jnp.int32, tile, 1) - lax.broadcasted_iota(
            jnp.int32, tile, 0
        )
        zeros = jnp.zeros(tile, jnp.float32)

        def add_rows(lo, hi, acc):
            for r in range(lo, hi, _SUBLANES):
                blk = xv[pl.ds(r, _SUBLANES), :]
                cols = [blk[:, c:c + _LANES] for c in range(0, n, _LANES)]
                while len(cols) > 1:
                    cols = [a + b for a, b in zip(cols[::2], cols[1::2])]
                sums = jnp.sum(cols[0], axis=1, keepdims=True)
                acc = jnp.where(diag == r % _LANES, sums, acc)
            return acc

        def fold(acc):
            return jnp.sum(acc, axis=0, keepdims=True)

        for g in range(groups - 1):
            loads[g].wait()
            if g == groups - 2:
                hop_out.wait()
                part[pl.ds(0, 1), :] = fold(add_rows(0, _DETOUR_ROWS, first))
            acc = add_rows(*chunks[g], zeros)
            if g == 0:
                first = acc
            else:
                part[pl.ds(g, 1), :] = fold(acc)
            if g == 1:
                hop_in.wait()
                hop_out.start()
        pl.semaphore_wait(barrier, 1)
        msg_head.start()

        loads[groups - 1].wait()
        acc = add_rows(*chunks[groups - 1], zeros)
        part[last, :] = fold(acc)
        msg_last.start()

        loads[groups].wait()
        mine_last = fold(add_rows(*chunks[groups], acc))
        tail[...] = mine_last
        msg_tail.start()

        msg_head.wait_send()
        msg_last.wait_send()
        msg_tail.wait_send()
        msg_head.wait_recv()
        out_ref[head, :] = (part[head, :] + recv[head, :]) * scale
        msg_last.wait_recv()
        theirs = recv[last, :]
        lane = lax.broadcasted_iota(jnp.int32, (1, _LANES), 1)
        msg_tail.wait_recv()
        for j in range(_LANES - _TAIL_ROWS, _LANES):
            theirs = jnp.where(lane == j, recv_tail[0, j], theirs)
        out_ref[last, :] = (mine_last + theirs) * scale

    out = pl.pallas_call(
        body,
        out_shape=jax.ShapeDtypeStruct((groups, _LANES), jnp.float32),
        in_specs=[pl.BlockSpec(memory_space=pl.ANY)],
        out_specs=pl.BlockSpec(memory_space=pltpu.VMEM),
        scratch_shapes=[
            pltpu.VMEM((m, n), jnp.float32),
            pltpu.SMEM((_DETOUR_ROWS, n), jnp.float32),
            pltpu.VMEM((groups, _LANES), jnp.float32),
            pltpu.VMEM((1, _LANES), jnp.float32),
            pltpu.VMEM((groups, _LANES), jnp.float32),
            pltpu.SMEM((1, _LANES), jnp.float32),
            pltpu.SemaphoreType.DMA((len(chunks),)),
            pltpu.SemaphoreType.DMA((2,)),
            pltpu.SemaphoreType.DMA((3,)),
            pltpu.SemaphoreType.DMA((3,)),
        ],
        compiler_params=pltpu.CompilerParams(
            collective_id=0,
            disable_bounds_checks=True,
            disable_semaphore_checks=True,
        ),
    )(x)
    return out.reshape(m, 1)
```

```python
import jax
import jax.numpy as jnp
from jax import lax
from jax.experimental import pallas as pl
from jax.experimental.pallas import tpu as pltpu

_LANES = 128
_SUBLANES = 8
_Y_SIZE = 2
_DETOUR_ROWS = 24
_DETOUR_TURN = 2
_TAIL_ROWS = 48


def pallas_dist_mean_ax1_xy_m1024_n512_kernel(x: jax.Array):
    m, n = x.shape
    groups = m // _LANES
    scale = 1.0 / (_Y_SIZE * n)
    detour_lo = _LANES - _DETOUR_ROWS
    cuts = [*range(_LANES, m, _LANES), m - _TAIL_ROWS, m]
    chunks = [(0, detour_lo), *zip(cuts[:-1], cuts[1:])]

    def body(x_hbm, out_ref, xv, hop, head, last, tail, peer_head, peer_last, peer_tail,
             load_sems, hop_sems, send_sems, recv_sems):
        def rows_of(ref, lo, hi):
            return ref.at[pl.ds(lo, hi - lo)]

        loads = [
            pltpu.make_async_copy(
                rows_of(x_hbm, lo, hi), rows_of(xv, lo, hi), load_sems.at[i]
            )
            for i, (lo, hi) in enumerate(chunks)
        ]
        hop_in = pltpu.make_async_copy(
            rows_of(x_hbm, detour_lo, _LANES), hop, hop_sems.at[0]
        )
        hop_out = pltpu.make_async_copy(
            hop, rows_of(xv, detour_lo, _LANES), hop_sems.at[1]
        )
        loads[0].start()
        hop_in.start()
        for load in loads[1:]:
            load.start()

        peer = (lax.axis_index("x"), 1 - lax.axis_index("y"))
        barrier = pltpu.get_barrier_semaphore()
        pl.semaphore_signal(
            barrier, 1, device_id=peer, device_id_type=pl.DeviceIdType.MESH
        )

        def to_peer(i, src, dst):
            return pltpu.make_async_remote_copy(
                src, dst, send_sems.at[i], recv_sems.at[i],
                device_id=peer, device_id_type=pl.DeviceIdType.MESH,
            )

        send_head = to_peer(0, head, peer_head)
        send_last = to_peer(1, last, peer_last)
        send_tail = to_peer(2, tail, peer_tail)

        tile = (_SUBLANES, _LANES)
        sublane = lax.broadcasted_iota(jnp.int32, tile, 0)
        lane = lax.broadcasted_iota(jnp.int32, tile, 1)
        zeros = jnp.zeros(tile, jnp.float32)

        def row_sums(lo, hi):
            sums = []
            for r in range(lo, hi, _SUBLANES):
                blk = xv[pl.ds(r, _SUBLANES), :]
                cols = [blk[:, c:c + _LANES] for c in range(0, n, _LANES)]
                while len(cols) > 1:
                    cols = [a + b for a, b in zip(cols[::2], cols[1::2], strict=True)]
                sums.append((r, jnp.sum(cols[0], axis=1, keepdims=True)))
            return sums

        def scatter(sums, acc=zeros):
            for r, s in sums:
                acc = jnp.where(lane - sublane == r % _LANES, s, acc)
            return acc

        def fold(acc):
            return jnp.sum(acc, axis=0, keepdims=True)

        for g in range(groups - 1):
            loads[g].wait()
            if g == groups - 2:
                hop_out.wait()
                head[pl.ds(0, 1), :] = fold(scatter(row_sums(detour_lo, _LANES), first))
            if g == _DETOUR_TURN:
                hop_in.wait()
                hop_out.start()
            acc = scatter(row_sums(*chunks[g]))
            if g == 0:
                first = acc
            else:
                head[pl.ds(g, 1), :] = fold(acc)
        pl.semaphore_wait(barrier, 1)
        send_head.start()

        loads[groups - 1].wait()
        acc = scatter(row_sums(*chunks[groups - 1]))
        last[...] = fold(acc)
        send_last.start()

        loads[groups].wait()
        sums = row_sums(*chunks[groups])
        pairs = zeros
        for i, (_, s) in enumerate(sums):
            pairs = jnp.where(lane - (sublane >> 1) == i * _SUBLANES // 2, s, pairs)
        pairs = pairs[0:4] + pairs[4:8]
        pairs = pairs[0:2] + pairs[2:4]
        tail[...] = pltpu.bitcast(pairs.astype(jnp.bfloat16), jnp.int32)
        send_tail.start()
        tail_row = lax.broadcasted_iota(jnp.int32, (1, _LANES), 1) - (_LANES - _TAIL_ROWS)
        own = fold(scatter(sums, acc))
        own = jnp.where(tail_row >= 0, own.astype(jnp.bfloat16).astype(jnp.float32), own)

        send_head.wait_send()
        send_last.wait_send()
        send_tail.wait_send()
        send_head.wait_recv()
        out_ref[pl.ds(0, groups - 1), :] = (head[...] + peer_head[...]) * scale

        shift = jnp.where((tail_row >= 0) & ((tail_row & 1) == 0), 16, 0)
        keep = jnp.where(tail_row >= 0, jnp.int32(-0x10000), jnp.int32(-1))
        send_last.wait_recv()
        bits = lax.bitcast_convert_type(peer_last[...], jnp.int32)
        send_tail.wait_recv()
        for word in range(_TAIL_ROWS // 2):
            bits = jnp.where(tail_row >> 1 == word, peer_tail[0, word], bits)
        theirs = lax.bitcast_convert_type((bits << shift) & keep, jnp.float32)
        out_ref[pl.ds(groups - 1, 1), :] = (own + theirs) * scale

    out = pl.pallas_call(
        body,
        out_shape=jax.ShapeDtypeStruct((groups, _LANES), jnp.float32),
        in_specs=[pl.BlockSpec(memory_space=pl.ANY)],
        out_specs=pl.BlockSpec(memory_space=pltpu.VMEM),
        scratch_shapes=[
            pltpu.VMEM((m, n), jnp.float32),
            pltpu.SMEM((_DETOUR_ROWS, n), jnp.float32),
            pltpu.VMEM((groups - 1, _LANES), jnp.float32),
            pltpu.VMEM((1, _LANES), jnp.float32),
            pltpu.VMEM((1, _LANES), jnp.int32),
            pltpu.VMEM((groups - 1, _LANES), jnp.float32),
            pltpu.VMEM((1, _LANES), jnp.float32),
            pltpu.SMEM((1, _LANES), jnp.int32),
            pltpu.SemaphoreType.DMA((len(chunks),)),
            pltpu.SemaphoreType.DMA((2,)),
            pltpu.SemaphoreType.DMA((3,)),
            pltpu.SemaphoreType.DMA((3,)),
        ],
        compiler_params=pltpu.CompilerParams(
            collective_id=0, disable_semaphore_checks=True
        ),
    )(x)
    return out.reshape(m, 1)
```
